```python
import numpy as np

kernel_name = "dist_moe_cap_ep_outshard_n2048_d512_e8_h1024"

def setup_inputs():
    x = np.random.randn(2048, 512).astype(np.float32)
    router_W = np.random.randn(512, 32).astype(np.float32) * 0.1
    scores64 = x.astype(np.float64) @ router_W.astype(np.float64)
    route_idx = np.argsort(-scores64, axis=-1)[:, :1].astype(np.int32)
    expert_W = np.random.randn(32, 512, 1024).astype(np.float32) * 0.02
    return {"x": x, "router_W": router_W, "route_idx": route_idx, "expert_W": expert_W}

def reference(x, router_W, route_idx, expert_W):
    counts = np.zeros(32, dtype=np.int64)
    out = np.zeros((2048, 1024), dtype=np.float32)
    for i in range(2048):
        e = int(route_idx[i, 0])
        if counts[e] < 51:
            out[i] = x[i] @ expert_W[e]
            counts[e] += 1
    return out
```

```python
import jax
import jax.numpy as jnp
from jax import lax
from jax.experimental import pallas as pl
from jax.experimental.pallas import tpu as pltpu


def pallas_dist_moe_cap_ep_outshard_n2048_d512_e8_h1024_kernel(
x: jax.Array,
    router_W: jax.Array,
    route_idx: jax.Array,
    expert_W: jax.Array,
):
    N, D, H, EL, CAP, S, T = 2048, 512, 1024, 8, 51, 64, 512
    f32, bf16, i32 = jnp.float32, jnp.bfloat16, jnp.int32

    def body(idx_ref, x_hbm, w_hbm, out, wbuf, xs, res, zrow, tokv, keepv, cntv,
             tok_s, keep_s, cnt_s, wsem, gsem, msem, ssem, rsem, padb):
        my = lax.axis_index("i")
        wcp = [pltpu.make_async_copy(w_hbm.at[e], wbuf.at[e], wsem.at[e]) for e in range(EL)]
        [c.start(priority=1) for c in wcp]

        bar = pltpu.get_barrier_semaphore()
        for o_ in (1, 2, 3):
            pl.semaphore_signal(bar, inc=1, device_id=((my + o_) % 4,), device_id_type=pl.DeviceIdType.MESH)
        idx = idx_ref[...]
        B = 256
        oh = (lax.broadcasted_iota(i32, (32, N), 0) == idx).astype(f32)
        U = (lax.broadcasted_iota(i32, (B, B), 0) < lax.broadcasted_iota(i32, (B, B), 1)).astype(bf16)
        carry = jnp.zeros((32, 1), f32)

        def prefix(oh, reset):
            carry = jnp.zeros((oh.shape[0], 1), f32)
            rs, ends = [], []
            for b in range(N // B):
                o = oh[:, b * B:(b + 1) * B]
                rk = jnp.dot(o.astype(bf16), U, preferred_element_type=f32) + carry
                rs.append(jnp.sum(rk * o, axis=0, keepdims=True))
                carry = carry + jnp.sum(o, axis=1, keepdims=True)
                if b % 2 == 1:
                    ends.append(carry)
                    if reset:
                        carry = jnp.zeros_like(carry)
            return jnp.concatenate(rs, axis=1).astype(i32), ends
        r, e1 = prefix(oh, False)
        j, ends = prefix(((lax.broadcasted_iota(i32, (8, N), 0) == (idx >> 3)) & (r < CAP)).astype(f32), True)
        lane = lax.broadcasted_iota(i32, (8, 128), 1)
        kk = jnp.zeros((8, 128), f32)
        for d in range(4):
            kk = jnp.where(lane == d, ends[d], kk)
        keepv[...] = kk.astype(i32)
        cntv[...] = jnp.broadcast_to(jnp.minimum(e1[-1], CAP).astype(i32), (32, 128))
        kf = (r < CAP).astype(f32)
        km = jnp.where(my == 0, kf[:, :T], jnp.where(my == 1, kf[:, T:2 * T], jnp.where(
            my == 2, kf[:, 2 * T:3 * T], kf[:, 3 * T:])))
        kcol = jnp.broadcast_to(km, (128, T)).T > 0.5
        A = (lax.broadcasted_iota(i32, (S, N), 0) == r).astype(bf16)
        row = lax.broadcasted_iota(i32, (128, N), 0)
        t = lax.broadcasted_iota(i32, (128, N), 1)
        val = jnp.where(row < 8, t >> 4, jnp.where(row < 16, t & 15, j >> 4))
        Bt = jnp.where(((row & 7) == idx - my * EL) & (row < 24), val, 0).astype(f32).astype(bf16)
        tk = lax.dot_general(A, Bt, (((1,), (1,)), ((), ())), preferred_element_type=f32).astype(i32)
        tokv[...] = tk * 16 + pltpu.roll(tk, 120, 1) + pltpu.roll(tk, 112, 1) * 2048
        mc = [pltpu.make_async_copy(a, b_, msem.at[i]) for i, (a, b_) in
              enumerate(((tokv, tok_s), (keepv, keep_s), (cntv, cnt_s)))]
        for c in mc:
            c.start()
        for c in mc:
            c.wait()

        def tok(e, s):
            return tok_s[s, e] & 2047

        def rc(src, row_, g, d):
            return pltpu.make_async_remote_copy(src, zrow.at[pl.ds(row_, 1)], ssem, rsem.at[my, g],
                                                device_id=(d,), device_id_type=pl.DeviceIdType.MESH)

        def gather(e):
            def g(s, c):
                pltpu.make_async_copy(x_hbm.at[pl.ds(tok(e, s), 1)],
                                      xs.at[e, pl.ds(s, 1)], gsem.at[e]).start()
                return c
            lax.fori_loop(0, 56, g, 0, unroll=4)

        with jax.named_scope('g01'):
            gather(0)
            gather(1)
        for e in range(0):
            wcp[e].start(priority=1)
        with jax.named_scope('grest'):
            for e in range(2, EL):
                gather(e)

        padb[...] = jnp.zeros(padb.shape, i32)
        pl.semaphore_wait(bar, 3)
        n = jnp.int32(0)
        for d in range(4):
            k = keep_s[my, d]
            kp = (k + 15) & -16
            n = n + kp

            def pad(q, c, d=d):
                rc(padb.at[pl.ds(0, 1)], T + my * 16 + (q & 15), q >> 4, d).start()
                return c
            lax.fori_loop(k, kp, pad, 0)

        for e in range(EL):
            with jax.named_scope('wwait'):
                wcp[e].wait()
            pltpu.make_async_copy(xs.at[e, pl.ds(0, 56)], xs.at[e, pl.ds(0, 56)], gsem.at[e]).wait()
            y = jnp.dot(xs[e].astype(bf16), wbuf[e].astype(bf16), preferred_element_type=f32)
            y = lax.bitcast_convert_type(y.astype(bf16).astype(f32), i32)
            res[e] = (y[:, :D] & -65536) | lax.shift_right_logical(y[:, D:], 16)

            def snd(s, c, e=e):
                w = tok_s[s, e]
                rc(res.at[e, pl.ds(s, 1)], w & 511, w >> 11, (w >> 9) & 3).start()
                return c
            lax.fori_loop(0, cnt_s[my * EL + e, 0], snd, 0)
        def ws(i, c):
            pltpu.make_async_copy(zrow.at[pl.ds(0, 16)], zrow.at[pl.ds(0, 16)], ssem).wait()
            return c
        lax.fori_loop(0, n >> 4, ws, 0)
        for s_ in range(4):
            def wr(g, c, s_=s_):
                pltpu.make_async_copy(zrow.at[pl.ds(0, 16)], zrow.at[pl.ds(0, 16)], rsem.at[s_, g]).wait()
                return c
            lax.fori_loop(0, (keep_s[s_, my] + 15) >> 4, wr, 0)
        for c in range(4):
            v = zrow[0:T, c * 128:(c + 1) * 128]
            out[:, c * 128:(c + 1) * 128] = jnp.where(kcol, lax.bitcast_convert_type(v & -65536, f32), 0.0)
            out[:, D + c * 128:D + (c + 1) * 128] = jnp.where(kcol, lax.bitcast_convert_type(v << 16, f32), 0.0)

    DMA = pltpu.SemaphoreType.DMA
    return pl.pallas_call(
        body,
        out_shape=jax.ShapeDtypeStruct((T, H), f32),
        in_specs=[pl.BlockSpec(memory_space=pltpu.VMEM), pl.BlockSpec(memory_space=pl.ANY),
                  pl.BlockSpec(memory_space=pl.ANY)],
        out_specs=pl.BlockSpec(memory_space=pltpu.VMEM),
        scratch_shapes=[
            pltpu.VMEM((EL, D, H), f32), pltpu.VMEM((EL, S, D), f32), pltpu.VMEM((EL, S, D), i32),
            pltpu.VMEM((T + 64, D), i32), pltpu.VMEM((S, 128), i32), pltpu.VMEM((8, 128), i32),
            pltpu.VMEM((32, 128), i32),
            pltpu.SMEM((S, 128), i32), pltpu.SMEM((8, 128), i32), pltpu.SMEM((32, 128), i32),
            DMA((EL,)), DMA((EL,)), DMA((3,)), DMA, DMA((4, 26)), pltpu.VMEM((8, D), i32),
        ],
        compiler_params=pltpu.CompilerParams(collective_id=0, disable_bounds_checks=True, vmem_limit_bytes=64 * 1024 * 1024),
    )(route_idx.astype(i32).reshape(1, N), x, expert_W)
```
